```python
import numpy as np

kernel_name = "dist_layernorm_xy_m6144_n2048"

def setup_inputs():
    x = np.random.randn(12288, 4096).astype(np.float32)
    gamma = np.random.randn(4096).astype(np.float32)
    beta = np.random.randn(4096).astype(np.float32)
    return {"x": x, "gamma": gamma, "beta": beta}

def reference(x: np.ndarray, gamma: np.ndarray, beta: np.ndarray) -> np.ndarray:
    eps = 1e-5
    mean = np.mean(x, axis=1, keepdims=True)
    var = np.var(x, axis=1, keepdims=True)
    return gamma * (x - mean) / np.sqrt(var + eps) + beta
```

```python
import jax
import jax.numpy as jnp
from jax import lax
from jax.experimental import pallas as pl
from jax.experimental.pallas import tpu as pltpu

EPS = 1e-5
N_Y = 2
BIG = 256
SMALL = 64
LOOKAHEAD = 3


def pallas_dist_layernorm_xy_m6144_n2048_kernel(
    x: jax.Array,
    gamma: jax.Array,
    beta: jax.Array,
):
    m, n = x.shape
    nbig = m // BIG - 1
    nsmall = BIG // SMALL
    nslots = nbig + nsmall
    tail0 = nbig * BIG
    assert m % BIG == 0 and BIG % SMALL == 0 and SMALL % 8 == 0
    assert BIG // 8 <= 128 and LOOKAHEAD <= min(nbig, nsmall)

    g2 = gamma.reshape(1, n)
    b2 = beta.reshape(1, n)

    def body(x_hbm, g_ref, b_ref, o_ref, send_buf, recv_buf, read_sems, send_sems, recv_sems):
        my_x = lax.axis_index("x")
        my_y = lax.axis_index("y")
        partner = (my_x, 1 - my_y)

        def read(row0, size, slot):
            rows = pl.ds(row0, size)
            return pltpu.make_async_copy(x_hbm.at[rows], o_ref.at[rows], read_sems.at[slot])

        def read_big(c):
            return read(c * BIG, BIG, c)

        def read_small(j):
            return read(tail0 + j * SMALL, SMALL, nbig + j)

        def exchange(slot):
            return pltpu.make_async_remote_copy(
                src_ref=send_buf.at[slot],
                dst_ref=recv_buf.at[slot],
                send_sem=send_sems.at[slot],
                recv_sem=recv_sems.at[slot],
                device_id=partner,
                device_id_type=pl.DeviceIdType.MESH,
            )

        def make_stage(size):
            ng = size // 8
            lane = lax.broadcasted_iota(jnp.int32, (ng, 8, 128), 2)
            grp = lax.broadcasted_iota(jnp.int32, (ng, 8, 128), 0)
            sel = lane == grp

            def pack(col):
                c3 = jnp.broadcast_to(col, (ng, 8, 128))
                return jnp.sum(jnp.where(sel, c3, 0.0), axis=0)

            def unpack(p):
                p3 = jnp.broadcast_to(p[None], (ng, 8, 128))
                return jnp.sum(jnp.where(sel, p3, 0.0), axis=2, keepdims=True)

            def local_stats(row0, slot):
                x3 = o_ref[pl.ds(row0, size), :].reshape(ng, 8, n)
                mean_l = jnp.sum(x3, axis=2, keepdims=True) * (1.0 / n)
                d = x3 - mean_l
                m2_l = jnp.sum(d * d, axis=2, keepdims=True)
                send_buf[slot, 0:8, :] = pack(mean_l)
                send_buf[slot, 8:16, :] = pack(m2_l)

            def finish(row0, slot):
                exchange(slot).wait()
                ma = send_buf[slot, 0:8, :]
                m2a = send_buf[slot, 8:16, :]
                mb = recv_buf[slot, 0:8, :]
                m2b = recv_buf[slot, 8:16, :]
                delta = ma - mb
                mean_p = 0.5 * (ma + mb)
                m2_p = m2a + m2b + delta * delta * (n / 2.0)
                var_p = m2_p * (1.0 / (N_Y * n))
                rstd_p = lax.rsqrt(var_p + EPS)
                mean = unpack(mean_p)
                rstd = unpack(rstd_p)
                rows = pl.ds(row0, size)
                x3 = o_ref[rows, :].reshape(ng, 8, n)
                out3 = (x3 - mean) * rstd * g_ref[...][None] + b_ref[...][None]
                o_ref[rows, :] = out3.reshape(size, n)

            return local_stats, finish

        for c in range(LOOKAHEAD):
            read_big(c).start()

        barrier_sem = pltpu.get_barrier_semaphore()
        pl.semaphore_signal(
            barrier_sem, inc=1, device_id=partner,
            device_id_type=pl.DeviceIdType.MESH,
        )
        pl.semaphore_wait(barrier_sem, 1)

        stats_big, finish_big = make_stage(BIG)
        stats_small, finish_small = make_stage(SMALL)

        def big_step(c, carry):
            read_big(c).wait()

            @pl.when(c + LOOKAHEAD < nbig)
            def _():
                read_big(jnp.minimum(c + LOOKAHEAD, nbig - 1)).start()

            @pl.when(c + LOOKAHEAD >= nbig)
            def _():
                read_small(jnp.clip(c + LOOKAHEAD - nbig, 0, nsmall - 1)).start()

            stats_big(c * BIG, c)
            exchange(c).start()

            @pl.when(c > 0)
            def _():
                prev = jnp.maximum(c - 1, 0)
                finish_big(prev * BIG, prev)

            return carry

        lax.fori_loop(0, nbig, big_step, 0)

        for j in range(nsmall):
            read_small(j).wait()
            if j + LOOKAHEAD < nsmall:
                read_small(j + LOOKAHEAD).start()
            stats_small(tail0 + j * SMALL, nbig + j)
            exchange(nbig + j).start()
            if j == 0:
                finish_big((nbig - 1) * BIG, nbig - 1)

        for j in range(nsmall):
            finish_small(tail0 + j * SMALL, nbig + j)

    return pl.pallas_call(
        body,
        in_specs=[
            pl.BlockSpec(memory_space=pl.ANY),
            pl.BlockSpec((1, n), lambda: (0, 0)),
            pl.BlockSpec((1, n), lambda: (0, 0)),
        ],
        out_specs=pl.BlockSpec(memory_space=pltpu.VMEM),
        out_shape=jax.ShapeDtypeStruct((m, n), x.dtype),
        scratch_shapes=[
            pltpu.VMEM((nslots, 16, 128), jnp.float32),
            pltpu.VMEM((nslots, 16, 128), jnp.float32),
            pltpu.SemaphoreType.DMA((nslots,)),
            pltpu.SemaphoreType.DMA((nslots,)),
            pltpu.SemaphoreType.DMA((nslots,)),
        ],
        compiler_params=pltpu.CompilerParams(
            collective_id=0,
            vmem_limit_bytes=60 * 1024 * 1024,
        ),
    )(x, g2, b2)
```
